```python
import numpy as np

kernel_name = "dist_mean_ax0_xy_m1024_n512"

def setup_inputs():
    return {"x": np.random.randn(2048, 1024).astype(np.float32)}

def reference(x: np.ndarray) -> np.ndarray:
    return np.mean(x, axis=0, keepdims=True)
```

```python
import jax
import jax.numpy as jnp
from jax import lax
from jax.experimental import pallas as pl
from jax.experimental.pallas import tpu as pltpu

_NCHUNKS = 4


def pallas_dist_mean_ax0_xy_m1024_n512_kernel(x: jax.Array):
    m, n = x.shape
    rows = m // _NCHUNKS
    scale = 1.0 / (2 * m)

    def body(x_hbm, o_ref, buf, send_buf, recv_buf, ld_sems, send_sem, recv_sem):
        mx = lax.axis_index("x")
        my = lax.axis_index("y")
        nbr = (1 - mx, my)
        copies = [
            pltpu.make_async_copy(
                x_hbm.at[pl.ds(i * rows, rows)],
                buf.at[pl.ds(i * rows, rows)],
                ld_sems.at[i],
            )
            for i in range(_NCHUNKS)
        ]
        for c in copies:
            c.start()
        bsem = pltpu.get_barrier_semaphore()
        pl.semaphore_signal(
            bsem, inc=1, device_id=nbr, device_id_type=pl.DeviceIdType.MESH
        )
        acc = None
        for i in range(_NCHUNKS):
            copies[i].wait()
            blk = buf[pl.ds(i * rows, rows), :].reshape(rows // 8, 8, n)
            s = jnp.sum(blk, axis=0)
            acc = s if acc is None else acc + s
        part = jnp.sum(acc, axis=0, keepdims=True)
        send_buf[...] = part
        pl.semaphore_wait(bsem, 1)
        rdma = pltpu.make_async_remote_copy(
            send_buf, recv_buf, send_sem, recv_sem,
            device_id=nbr, device_id_type=pl.DeviceIdType.MESH,
        )
        rdma.start()
        rdma.wait_recv()
        o_ref[...] = (part + recv_buf[...]) * scale
        rdma.wait_send()

    return pl.pallas_call(
        body,
        out_shape=jax.ShapeDtypeStruct((1, n), x.dtype),
        in_specs=[pl.BlockSpec(memory_space=pl.ANY)],
        out_specs=pl.BlockSpec(memory_space=pltpu.VMEM),
        scratch_shapes=[
            pltpu.VMEM((m, n), jnp.float32),
            pltpu.VMEM((1, n), jnp.float32),
            pltpu.VMEM((1, n), jnp.float32),
            pltpu.SemaphoreType.DMA((_NCHUNKS,)),
            pltpu.SemaphoreType.DMA,
            pltpu.SemaphoreType.DMA,
        ],
        compiler_params=pltpu.CompilerParams(collective_id=0),
    )(x)
```

```python
import jax
import jax.numpy as jnp
from jax import lax
from jax.experimental import pallas as pl
from jax.experimental.pallas import tpu as pltpu

_SUBLANES = 8


def _row_chunks(m):
    if m % 32 == 0 and m >= 256:
        tail = (3 * m // 32, m // 32)
        if all(t % _SUBLANES == 0 for t in tail):
            return (m - sum(tail),) + tail
    return (m,)


def _sum_rows(ref, start, rows, n):
    if rows % _SUBLANES:
        return jnp.pad(
            jnp.sum(ref[pl.ds(start, rows), :], axis=0, keepdims=True),
            ((0, _SUBLANES - 1), (0, 0)),
        )
    groups = rows // _SUBLANES
    chains = 2 if groups % 2 == 0 and groups >= 4 else 1
    per = groups // chains
    acc = None
    for c in range(chains):
        blk = ref[pl.ds(start + c * per * _SUBLANES, per * _SUBLANES), :]
        s = jnp.sum(blk.reshape(per, _SUBLANES, n), axis=0)
        acc = s if acc is None else acc + s
    return acc


def pallas_dist_mean_ax0_xy_m1024_n512_kernel(x: jax.Array):
    m, n = x.shape
    chunks = _row_chunks(m)
    starts = tuple(sum(chunks[:i]) for i in range(len(chunks)))
    scale = 1.0 / (2 * m)

    def body(x_hbm, o_ref, buf, send_buf, recv_buf, load_sems, send_sem, recv_sem):
        loads = [
            pltpu.make_async_copy(
                x_hbm.at[pl.ds(starts[i], chunks[i])],
                buf.at[pl.ds(starts[i], chunks[i])],
                load_sems.at[i],
            )
            for i in range(len(chunks))
        ]
        for load in loads:
            load.start()

        neighbour = (1 - lax.axis_index("x"), lax.axis_index("y"))
        barrier = pltpu.get_barrier_semaphore()
        pl.semaphore_signal(
            barrier, inc=1, device_id=neighbour,
            device_id_type=pl.DeviceIdType.MESH,
        )

        acc = None
        for i, load in enumerate(loads):
            if i == len(loads) - 1:
                pl.semaphore_wait(barrier, 1)
            load.wait()
            s = _sum_rows(buf, starts[i], chunks[i], n)
            acc = s if acc is None else acc + s
        send_buf[...] = jnp.sum(acc, axis=0, keepdims=True) * scale

        swap = pltpu.make_async_remote_copy(
            src_ref=send_buf, dst_ref=recv_buf,
            send_sem=send_sem, recv_sem=recv_sem,
            device_id=neighbour, device_id_type=pl.DeviceIdType.MESH,
        )
        swap.start()
        swap.wait_recv()
        o_ref[...] = (send_buf[...] + recv_buf[...]).astype(o_ref.dtype)
        swap.wait_send()

    return pl.pallas_call(
        body,
        out_shape=jax.ShapeDtypeStruct((1, n), x.dtype),
        in_specs=[pl.BlockSpec(memory_space=pl.ANY)],
        out_specs=pl.BlockSpec(memory_space=pltpu.VMEM),
        scratch_shapes=[
            pltpu.VMEM((m, n), x.dtype),
            pltpu.VMEM((1, n), jnp.float32),
            pltpu.VMEM((1, n), jnp.float32),
            pltpu.SemaphoreType.DMA((len(chunks),)),
            pltpu.SemaphoreType.DMA,
            pltpu.SemaphoreType.DMA,
        ],
        compiler_params=pltpu.CompilerParams(
            collective_id=0,
            disable_semaphore_checks=True,
        ),
    )(x)
```

```python
import jax
import jax.numpy as jnp
from jax import lax
from jax.experimental import pallas as pl
from jax.experimental.pallas import tpu as pltpu

_SUBLANES = 8


def _row_chunks(m):
    assert m % (32 * _SUBLANES) == 0, m
    return (28 * m // 32, 3 * m // 32, m // 32)


def _sum_rows(ref, start, rows, n):
    groups = rows // _SUBLANES
    chains = 2 if groups % 2 == 0 and groups >= 4 else 1
    per = groups // chains
    acc = None
    for c in range(chains):
        blk = ref[pl.ds(start + c * per * _SUBLANES, per * _SUBLANES), :]
        s = jnp.sum(blk.reshape(per, _SUBLANES, n), axis=0)
        acc = s if acc is None else acc + s
    return acc


def pallas_dist_mean_ax0_xy_m1024_n512_kernel(x: jax.Array):
    m, n = x.shape
    chunks = _row_chunks(m)
    starts = tuple(sum(chunks[:i]) for i in range(len(chunks)))
    scale = 1.0 / (2 * m)

    def body(x_hbm, o_ref, buf, send_buf, recv_buf, load_sems, send_sem, recv_sem):
        loads = [
            pltpu.make_async_copy(
                x_hbm.at[pl.ds(starts[i], chunks[i])],
                buf.at[pl.ds(starts[i], chunks[i])],
                load_sems.at[i],
            )
            for i in range(len(chunks))
        ]
        for load in loads:
            load.start()

        neighbour = (1 - lax.axis_index("x"), lax.axis_index("y"))
        barrier = pltpu.get_barrier_semaphore()
        pl.semaphore_signal(
            barrier, inc=1, device_id=neighbour,
            device_id_type=pl.DeviceIdType.MESH,
        )

        acc = None
        for i, load in enumerate(loads):
            if i == len(loads) - 1:
                pl.semaphore_wait(barrier, 1)
            load.wait()
            s = _sum_rows(buf, starts[i], chunks[i], n)
            acc = s if acc is None else acc + s
        send_buf[...] = jnp.sum(acc, axis=0, keepdims=True) * scale

        swap = pltpu.make_async_remote_copy(
            src_ref=send_buf, dst_ref=recv_buf,
            send_sem=send_sem, recv_sem=recv_sem,
            device_id=neighbour, device_id_type=pl.DeviceIdType.MESH,
        )
        swap.start()
        swap.wait_recv()
        o_ref[...] = (send_buf[...] + recv_buf[...]).astype(o_ref.dtype)
        swap.wait_send()

    return pl.pallas_call(
        body,
        out_shape=jax.ShapeDtypeStruct((1, n), x.dtype),
        in_specs=[pl.BlockSpec(memory_space=pl.ANY)],
        out_specs=pl.BlockSpec(memory_space=pltpu.VMEM),
        scratch_shapes=[
            pltpu.VMEM((m, n), x.dtype),
            pltpu.VMEM((1, n), jnp.float32),
            pltpu.VMEM((1, n), jnp.float32),
            pltpu.SemaphoreType.DMA((len(chunks),)),
            pltpu.SemaphoreType.DMA,
            pltpu.SemaphoreType.DMA,
        ],
        compiler_params=pltpu.CompilerParams(
            collective_id=0,
            disable_semaphore_checks=True,
        ),
    )(x)
```
